```python
import numpy as np

kernel_name = "dist_sort_i_m128_n64"

def setup_inputs():
    return {"x": np.random.randn(512, 64).astype(np.float32)}

def reference(x: np.ndarray) -> np.ndarray:
    return np.sort(x, axis=0)
```

```python
import jax
import jax.numpy as jnp
from jax import lax
from jax.experimental import pallas as pl
from jax.experimental.pallas import tpu as pltpu

_VREG = (8, 128)
_F32 = jnp.float32
_BF16 = jnp.bfloat16

_NET16 = (
    ((0, 1), (2, 3), (4, 5), (6, 7), (8, 9), (10, 11), (12, 13), (14, 15)),
    ((0, 2), (1, 3), (4, 6), (5, 7), (8, 10), (9, 11), (12, 14), (13, 15)),
    ((0, 4), (1, 5), (2, 6), (3, 7), (8, 12), (9, 13), (10, 14), (11, 15)),
    ((0, 8), (1, 9), (2, 10), (3, 11), (4, 12), (5, 13), (6, 14), (7, 15)),
    ((5, 10), (6, 9), (3, 12), (13, 14), (7, 11), (1, 2), (4, 8)),
    ((1, 4), (7, 13), (2, 8), (11, 14), (5, 6), (9, 10)),
    ((2, 4), (11, 13), (3, 8), (7, 12)),
    ((6, 8), (10, 12), (3, 5), (7, 9)),
    ((3, 4), (5, 6), (7, 8), (9, 10), (11, 12)),
    ((6, 7), (8, 9)),
)


def _parity(v):
    return bin(v).count("1") & 1


def _gather(x, idx, axis):
    dn = lax.GatherDimensionNumbers(
        offset_dims=(),
        collapsed_slice_dims=(axis,),
        start_index_map=(axis,),
        operand_batching_dims=(1 - axis,),
        start_indices_batching_dims=(1 - axis,),
    )
    return lax.gather(x, idx[..., None], dn, (1, 1),
                      mode=lax.GatherScatterMode.PROMISE_IN_BOUNDS)


class _Geometry:
    def __init__(self):
        self.sub = lax.broadcasted_iota(jnp.int32, _VREG, 0)
        self.lane = lax.broadcasted_iota(jnp.int32, _VREG, 1)

    def flip(self, x, d):
        if d == 4:
            return pltpu.roll(x, 4, 0)
        return _gather(x, self.sub ^ d, 0)

    def table(self, values):
        word = sum(v << (3 * s) for s, v in enumerate(values))
        return (jnp.full(_VREG, word, jnp.int32) >> (3 * self.sub)) & 7

    def sub_bit(self, f):
        word = sum(_parity(s & f) << s for s in range(8))
        return (jnp.full(_VREG, word, jnp.int32) >> self.sub) & 1

    def lane_bit(self, b):
        return (self.lane >> b) & 1


def _ce(a, b):
    return jnp.minimum(a, b), jnp.maximum(a, b)


def _merge_lists(a, b):
    if len(a) == 1:
        return list(_ce(a[0], b[0]))
    even = _merge_lists(a[0::2], b[0::2])
    odd = _merge_lists(a[1::2], b[1::2])
    out = [even[0]]
    for i in range(len(odd) - 1):
        out += _ce(odd[i], even[i + 1])
    return out + [odd[-1]]


def _partner(flipped, kept):
    return min(d for d in range(1, 8)
               if all(_parity(d & f) for f in flipped)
               and not any(_parity(d & f) for f in kept))


def _stage(x, bit):
    x = list(x)
    for i in range(len(x)):
        if not i >> bit & 1:
            j = i | 1 << bit
            x[i], x[j] = _ce(x[i], x[j])
    return x


def _cond_swap(x, bit, keep):
    x = list(x)
    for i in range(len(x)):
        if not i >> bit & 1:
            j = i | 1 << bit
            x[i], x[j] = jnp.where(keep, x[i], x[j]), jnp.where(keep, x[j], x[i])
    return x


def _sublane_stage(g, x, bit, keep, d):
    x = _cond_swap(x, bit, keep)
    x = [g.flip(v, d) if i >> bit & 1 else v for i, v in enumerate(x)]
    return _stage(x, bit)


_FUNS = (7, 3, 1)
_SORTED = ((0, 4, 5, 6), (3, 2, 1))


def _sort128(g, x):
    x = list(x)
    for layer in _NET16:
        for i, j in layer:
            x[i], x[j] = _ce(x[i], x[j])
    funs = []
    for k, t in enumerate((4, 2, 1)):
        rest = list((4, 2, 1)[k + 1:])
        d = _partner(funs + [t], rest)
        x = _merge_lists(x[0::2], [g.flip(v, d) for v in x[1::2]])
        funs = [f ^ t for f in funs] + [t]
        for f in funs:
            d = _partner([f], [h for h in funs if h != f] + rest)
            x = _sublane_stage(g, x, 0, g.sub_bit(f) == 0, d)
    assert tuple(funs) == _FUNS
    return x


def _step(f):
    return _partner([f], [h for h in _FUNS if h != f])


def _reversed(g, x, have, want):
    src = []
    for s in range(8):
        t = 0
        for f, r in zip(_FUNS, want[1]):
            if not _parity(s & f):
                t ^= _step(_FUNS[have[1].index(r)])
        src.append(t)
    idx = g.table(src)
    out = []
    for i in range(len(x)):
        j = sum((~i >> b & 1) << have[0].index(r) for b, r in enumerate(want[0]))
        out.append(_gather(x[j], idx, 0))
    return out


def _bitonic(g, x, layout, work, twist=False):
    list_bits, sub_bits = list(layout[0]), list(layout[1])
    for r in sorted(list_bits + sub_bits, reverse=True):
        if r in list_bits:
            x = _stage(x, list_bits.index(r))
        else:
            n = sub_bits.index(r)
            keep = g.sub_bit(_FUNS[n]) == (g.lane_bit(n) if twist else 0)
            x = _sublane_stage(g, x, work, keep, _step(_FUNS[n]))
            list_bits[work], sub_bits[n] = r, list_bits[work]
    return x, (tuple(list_bits), tuple(sub_bits))


def _skew4(g, x):
    t = g.sub + g.lane
    p = [_gather(v, t & 7, 0) for v in x]
    for b in range(2):
        on = (t >> (3 + b)) & 1 == 1
        p = [jnp.where(on, p[(j + (1 << b)) % 4], p[j]) for j in range(4)]
    return p


def _spread(g, lo, hi):
    k = (g.sub + g.lane) >> 3
    q = [None] * 8
    for j in range(4):
        first = (k + j) & 4 == 0
        q[j] = jnp.where(first, lo[j], hi[j])
        q[j + 4] = jnp.where(first, hi[j], lo[j])
    return [pltpu.roll(q[t % 8], 8 * t, 1, stride=1, stride_axis=0)
            for j in range(4) for t in (j, j + 8, j + 4, j + 12)]


def _finish(g, y, layout, work, o_ref):
    y, (list_bits, sub_bits) = _bitonic(g, y, layout, work, twist=True)
    for i in range(3):
        y = _cond_swap(y, i, g.lane_bit(3 + i) == 0)
    src = g.lane & 64
    back = 0
    for n in range(3):
        src |= (g.lane_bit(sub_bits[n]) ^ g.sub_bit(_FUNS[n])) << n
        src |= g.lane_bit(list_bits[n]) << (3 + n)
        back ^= (g.lane_bit(sub_bits[n]) ^ ((g.sub >> n) & 1)) * _step(_FUNS[n])
    z = [_gather(_gather(y[v], src ^ (v << 3), 1), back, 0) for v in range(8)]
    for i in range(3):
        z = _cond_swap(z, i, g.lane_bit(list_bits[i]) == 0)
    for v in range(8):
        o_ref[8 * v:8 * v + 8, :] = z[v]


def _rows(ref, n, first=0):
    return [ref[first + 8 * j:first + 8 * j + 8, :].astype(_F32) for j in range(n)]


def _body(x_hbm, o_ref, x_vmem, mine, runs, raw, rest_out, rest_in,
          in_sems, send_sems, recv_sems, hello):
    me = lax.axis_index("i")
    load_hi = pltpu.make_async_copy(
        x_hbm.at[pl.ds(32, 32)], x_vmem.at[pl.ds(32, 32)], in_sems.at[0])
    load_lo = pltpu.make_async_copy(
        x_hbm.at[pl.ds(0, 32)], x_vmem.at[pl.ds(0, 32)], in_sems.at[1])
    barrier = pltpu.get_barrier_semaphore()

    def remote(src, dst, k, to):
        return pltpu.make_async_remote_copy(
            src, dst, send_sems.at[k], recv_sems.at[k],
            device_id=to, device_id_type=pl.DeviceIdType.LOGICAL)

    def run_copy(slot, to):
        return remote(mine, runs.at[slot], slot, to)

    def signal(sem, to):
        pl.semaphore_signal(sem, inc=1, device_id=to,
                            device_id_type=pl.DeviceIdType.LOGICAL)

    raw_copy = lambda: remote(x_hbm.at[pl.ds(0, 32)], raw, 3, 0)
    rest_copy = lambda: remote(rest_out, rest_in, 4, 0)

    load_hi.start()

    @pl.when(me == 2)
    def _():
        pl.semaphore_wait(barrier, 1)
        raw_copy().start()
        signal(hello, 0)

    load_lo.start()

    @pl.when(me == 0)
    def _():
        for to in (2, 1, 3):
            signal(barrier, to)

    @pl.when(me % 2 == 1)
    def _():
        signal(barrier, 0)

    g = _Geometry()
    load_hi.wait()
    hi = _skew4(g, _rows(x_vmem, 4, 32))
    for j in range(4):
        rest_out[8 * j:8 * j + 8, :] = hi[j].astype(_BF16)

    @pl.when(me == 2)
    def _():
        rest_copy().start()

    load_lo.wait()
    own = _sort128(g, _spread(g, _skew4(g, _rows(x_vmem, 4)), hi))
    low_half = g.lane < 64
    for j in range(8):
        mine[8 * j:8 * j + 8, :] = jnp.where(low_half, own[j], own[j + 8]).astype(_BF16)

    def run(slot):
        w = _rows(runs.at[slot], 8)
        r = [pltpu.roll(v, 64, 1) for v in w]
        return ([jnp.where(low_half, a, b) for a, b in zip(w, r)]
                + [jnp.where(low_half, b, a) for a, b in zip(w, r)])

    @pl.when(me == 0)
    def _():
        pl.semaphore_wait(barrier, 2)
        for to in (2, 1, 3):
            signal(barrier, to)
        run_copy(0, 1).start()
        run_copy(2, 3).start()
        pl.semaphore_wait(hello, 1)
        for to in (1, 3):
            signal(barrier, to)
        run_copy(1, 2).start()
        run_copy(0, 0).wait_recv()
        run_copy(2, 0).wait_recv()
        m, layout = own, _SORTED
        for slot in (0, 2):
            m = _reversed(g, m, layout, _SORTED)
            m = [jnp.minimum(a, b) for a, b in zip(m, run(slot))]
            m, layout = _bitonic(g, m, _SORTED, 0)
        m = _reversed(g, m, layout, _SORTED)
        near = [jnp.where(low_half, m[i + 8], m[i]) for i in range(8)]
        far = [jnp.where(low_half, -jnp.inf, m[i + 8]) for i in range(8)]
        for slot in range(3):
            run_copy(slot, 0).wait_send()
        raw_copy().wait_recv()
        lo = _skew4(g, _rows(raw, 4))
        rest_copy().wait_recv()
        t = _sort128(g, _spread(g, lo, _rows(rest_in, 4)))
        y = [jnp.maximum(jnp.minimum(near[i], t[i]), jnp.minimum(far[i], t[i + 8]))
             for i in range(8)]
        _finish(g, y, (_SORTED[0][:3], _SORTED[1]), 1, o_ref)

    @pl.when(me != 0)
    def _():
        @pl.when(me == 2)
        def _():
            pl.semaphore_wait(barrier, 1)
            run_copy(0, 3).start()
            run_copy(2, 1).start()
            raw_copy().wait_send()
            rest_copy().wait_send()

        @pl.when(me != 2)
        def _():
            pl.semaphore_wait(barrier, 1)
            run_copy(3 - me, 0).start()
            pl.semaphore_wait(barrier, 1)
            run_copy(1, 4 - me).start()
            pl.semaphore_wait(barrier, 1)
            run_copy(me - 1, 2).start()
            run_copy(1, 0).wait_send()

        run_copy(0, 0).wait_send()
        run_copy(2, 0).wait_send()
        for slot in range(3):
            run_copy(slot, 0).wait_recv()

        def merge(a, b):
            pairs = [_ce(u, v) for u, v in zip(a, _reversed(g, b, _SORTED, _SORTED))]
            lo, layout = _bitonic(g, [p[0] for p in pairs], _SORTED, 1)
            hi, layout = _bitonic(g, [p[1] for p in pairs], _SORTED, 1)
            return lo, hi, layout

        def pick(lower, a, b):
            return [jnp.where(lower, *_ce(u, v)) for u, v in zip(a, b)]

        p_lo, p_hi, layout = merge(own, run(0))
        q_lo, q_hi, layout = merge(run(1), run(2))
        z = pick(me == 2,
                 pick(me == 1, p_lo, _reversed(g, q_hi, layout, layout)),
                 pick(me == 1, p_hi, _reversed(g, q_lo, layout, layout)))
        _finish(g, pick(low_half, z[:8], z[8:]), (layout[0][:3], layout[1]), 2, o_ref)


def pallas_dist_sort_i_m128_n64_kernel(x):
    out = pl.pallas_call(
        _body,
        out_shape=jax.ShapeDtypeStruct((64, 128), _F32),
        in_specs=[pl.BlockSpec(memory_space=pltpu.MemorySpace.HBM)],
        out_specs=pl.BlockSpec(memory_space=pltpu.MemorySpace.VMEM),
        scratch_shapes=[
            pltpu.VMEM((64, 128), _F32),
            pltpu.VMEM((64, 128), _BF16),
            pltpu.VMEM((3, 64, 128), _BF16),
            pltpu.VMEM((32, 128), _F32),
            pltpu.VMEM((32, 128), _BF16),
            pltpu.VMEM((32, 128), _BF16),
            pltpu.SemaphoreType.DMA((2,)),
            pltpu.SemaphoreType.DMA((5,)),
            pltpu.SemaphoreType.DMA((5,)),
            pltpu.SemaphoreType.REGULAR,
        ],
        compiler_params=pltpu.CompilerParams(
            collective_id=0,
            disable_bounds_checks=True,
            disable_semaphore_checks=True,
        ),
    )(x.T)
    return out.T
```

```python
import jax
import jax.numpy as jnp
from jax import lax
from jax.experimental import pallas as pl
from jax.experimental.pallas import tpu as pltpu

_VREG = (8, 128)
_F32 = jnp.float32
_BF16 = jnp.bfloat16


def _parity(v):
    return bin(v).count("1") & 1


def _partner(flipped, kept):
    return min(d for d in range(1, 8)
               if all(_parity(d & f) for f in flipped)
               and not any(_parity(d & f) for f in kept))


_FUNS = (7, 3, 1)
_STEPS = tuple(_partner([f], [h for h in _FUNS if h != f]) for f in _FUNS)
_SORTED = ((0, 4, 5, 6), (3, 2, 1))
_ARRIVAL = (4, 5, 0, 2, 1, 3, 6, 7, 8, 11, 9, 10, 14, 12, 13, 15)


def _gather(x, idx, axis):
    dims = lax.GatherDimensionNumbers(
        offset_dims=(),
        collapsed_slice_dims=(axis,),
        start_index_map=(axis,),
        operand_batching_dims=(1 - axis,),
        start_indices_batching_dims=(1 - axis,),
    )
    return lax.gather(x, idx[..., None], dims, (1, 1),
                      mode=lax.GatherScatterMode.PROMISE_IN_BOUNDS)


def _rotate(x, shift):
    return pltpu.roll(x, shift, 1, stride=1, stride_axis=0)


class _Geometry:
    def __init__(self):
        self.sub = lax.broadcasted_iota(jnp.int32, _VREG, 0)
        self.lane = lax.broadcasted_iota(jnp.int32, _VREG, 1)
        self.diag = self.sub + self.lane
        self.skew = self.diag & 7
        self.xor = {d: self.sub ^ d for d in _STEPS if d != 4}
        self.bits = {}
        for f in (4, 6, 2) + _FUNS:
            word = sum(_parity(s & f) << s for s in range(8))
            self.bits[f] = (jnp.full(_VREG, word, jnp.int32) >> self.sub) & 1

    def flip(self, x, d):
        if d == 4:
            return pltpu.roll(x, 4, 0)
        return _gather(x, self.xor[d], 0)

    def lane_bit(self, b):
        return (self.lane >> b) & 1

    def rows_from(self, have, want, invert):
        word = 0
        for s in range(8):
            for f, r in zip(_FUNS, want):
                step = _STEPS[have.index(r)]
                word ^= (_parity(s & f) ^ invert) * step << (3 * s)
        return (jnp.full(_VREG, word, jnp.int32) >> (3 * self.sub)) & 7


def _ce(a, b):
    return jnp.minimum(a, b), jnp.maximum(a, b)


def _merge_lists(a, b):
    if not a or not b:
        return list(a) + list(b)
    if len(a) == 1 and len(b) == 1:
        return list(_ce(a[0], b[0]))
    even = _merge_lists(a[0::2], b[0::2])
    odd = _merge_lists(a[1::2], b[1::2])
    n = min(len(odd), len(even) - 1)
    out = [even[0]]
    for i in range(n):
        out += _ce(odd[i], even[i + 1])
    return out + odd[n:] + even[n + 1:]


def _sort_list(x):
    if len(x) < 2:
        return list(x)
    half = len(x) // 2
    return _merge_lists(_sort_list(x[:half]), _sort_list(x[half:]))


def _by_arrival(x):
    return [x[i] for i in _ARRIVAL if i < len(x)]


def _sort_vregs(x):
    x = _by_arrival(x)
    early = _merge_lists(_sort_list(x[:8]), _sort_list(x[8:12]))
    return _merge_lists(early, _sort_list(x[12:]))


def _on_pairs(x, bit, fn):
    x = list(x)
    for i in range(len(x)):
        if not i >> bit & 1:
            j = i | 1 << bit
            x[i], x[j] = fn(x[i], x[j])
    return x


def _stage(x, bit, down=False):
    return _on_pairs(x, bit, lambda a, b: _ce(a, b)[::-1 if down else 1])


def _cond_swap(x, bit, keep):
    return _on_pairs(x, bit, lambda a, b: (jnp.where(keep, a, b),
                                           jnp.where(keep, b, a)))


def _sublane_stage(g, x, bit, keep, d, down=False):
    x = _cond_swap(x, bit, keep)
    x = [g.flip(v, d) if i >> bit & 1 else v for i, v in enumerate(x)]
    return _stage(x, bit, down)


def _level(level):
    order = (4, 2, 1)
    funs = []
    for u in order[:level]:
        funs = [f ^ u for f in funs] + [u]
    return funs, order[level], list(order[level + 1:])


def _merge_classes(g, x, level):
    funs, t, rest = _level(level)
    d = _partner(funs + [t], rest)
    return _merge_lists(x[0::2], [g.flip(v, d) for v in x[1::2]])


def _tidy(g, x, level, lower=None):
    funs, t, rest = _level(level)
    funs = [f ^ t for f in funs] + [t]
    for n, f in enumerate(funs):
        d = _partner([f], [h for h in funs if h != f] + rest)
        x = _sublane_stage(g, x, 0, g.bits[f] == 0, d)
        if lower is not None:
            x = [jnp.where(lower[n], a, b) for a, b in zip(x[0::2], x[1::2])]
    return x


def _merge_sublanes(g, x, lo=0, hi=6):
    for step in range(lo, hi):
        x = (_tidy if step % 2 else _merge_classes)(g, x, step // 2)
    return x


def _reversed(x, rows):
    return [_gather(v, rows, 0) for v in x[::-1]]


def _final_layout(layout, work):
    list_bits, sub_bits = list(layout[0]), list(layout[1])
    for r in sorted(list_bits + sub_bits, reverse=True):
        if r not in list_bits:
            n = sub_bits.index(r)
            list_bits[work], sub_bits[n] = r, list_bits[work]
    return tuple(list_bits), tuple(sub_bits)


def _bitonic(g, x, layout, work, keep=None, down=False):
    list_bits, sub_bits = list(layout[0]), list(layout[1])
    for r in sorted(list_bits + sub_bits, reverse=True):
        if r in list_bits:
            x = _stage(x, list_bits.index(r), down)
        else:
            n = sub_bits.index(r)
            k = g.bits[_FUNS[n]] == 0 if keep is None else keep[n]
            x = _sublane_stage(g, x, work, k, _STEPS[n], down)
            list_bits[work], sub_bits[n] = r, list_bits[work]
    return x


def _quarter(run, bound):
    out = []
    for i, b in enumerate(bound):
        c = [b[0]] + [jnp.maximum(v, b[j]) if j < len(b) else v
                      for j, v in enumerate(run[i::4], 1)]
        while len(c) > 1:
            if len(c) % 2:
                c = c[1:-1] + [jnp.minimum(c[0], c[-1])]
            else:
                c = [jnp.minimum(p, q) for p, q in zip(c[0::2], c[1::2])]
        out.append(c[0])
    return out


def _barrel(p, masks):
    n = len(p)
    for b, on in enumerate(masks):
        p = [jnp.where(on, p[(j + (1 << b)) % n], p[j]) for j in range(n)]
    return p


def _skew(g, x):
    masks = [(g.diag >> (3 + b)) & 1 == 1
             for b in range(len(x).bit_length() - 1)]
    return _barrel([_gather(v, g.skew, 0) for v in x], masks)


class _SkewOfThree:
    def __init__(self, g):
        self.g = g
        k = ((g.diag >> 3) + 3) & 3
        self.at = [k == j for j in range(4)]

    def fold(self, x):
        p, at = [_gather(v, self.g.skew, 0) for v in x], self.at
        return [jnp.where(at[1], p[1], jnp.where(at[0], p[0], p[2])),
                jnp.where(at[1], p[2], jnp.where(at[3], p[0], p[1])),
                jnp.where(at[3], p[1], jnp.where(at[0], p[2], p[0]))]

    def unfold(self, w, missing, j):
        if j == 3:
            v = jnp.where(self.at[1], w[2], jnp.where(self.at[2], w[1], w[0]))
        else:
            v = w[j]
        return jnp.where(self.at[3 - j], missing, v)


def _spread(q, n, first=0):
    return [_rotate(v, 8 * t)
            for j, v in enumerate(q, first) for t in range(j, 16, n)]


class _Exit:
    def __init__(self, g, layout, work):
        self.g, self.layout, self.work = g, layout, work
        self.list_bits, sub_bits = _final_layout(layout, work)
        n = len(self.list_bits)
        src = g.lane & (128 - (8 << n))
        back = 0
        for i in range(3):
            src |= (g.lane_bit(sub_bits[i]) ^ g.bits[_FUNS[i]]) << i
            back ^= (g.lane_bit(sub_bits[i]) ^ ((g.sub >> i) & 1)) * _STEPS[i]
        for i in range(n):
            src |= g.lane_bit(self.list_bits[i]) << (3 + i)
        self.src = [src ^ (v << 3) for v in range(1 << n)]
        self.back = back
        self.sub_twist = [g.lane_bit(i) for i in range(3)]
        self.list_twist = [g.lane_bit(3 + i) for i in range(n)]

    def sort(self, y):
        keep = [self.g.bits[f] == v for f, v in zip(_FUNS, self.sub_twist)]
        y = _bitonic(self.g, y, self.layout, self.work, keep)
        for i, v in enumerate(self.list_twist):
            y = _cond_swap(y, i, v == 0)
        return y

    def cross(self, y):
        return [_gather(v, src, 1) for v, src in zip(y, self.src)]

    def untwist(self, z):
        z = [_gather(v, self.back, 0) for v in z]
        for i, r in enumerate(self.list_bits):
            z = _cond_swap(z, i, self.g.lane_bit(r) == 0)
        return z


def _rows(ref, n, first=0):
    return [ref[8 * j:8 * j + 8, :].astype(_F32)
            for j in range(first, first + n)]


def _put(ref, x, first=0):
    for j, v in enumerate(x, first):
        ref[8 * j:8 * j + 8, :] = v.astype(ref.dtype)


def _body(x_hbm, o_ref, x_vmem, near, mine, runs, raw, edge, head_out, head_in,
          mid_out, mid_in, top_out, top_in, in_sems, send_sems, recv_sems,
          odd_here, far_here):
    me = lax.axis_index("i")
    loads = [
        pltpu.make_async_copy(x_hbm.at[rows], x_vmem.at[rows], in_sems.at[k])
        for k, rows in enumerate((pl.ds(40, 24), pl.ds(0, 16), pl.ds(16, 24)))
    ]
    barrier = pltpu.get_barrier_semaphore()

    def signal(sem, to):
        pl.semaphore_signal(sem, inc=1, device_id=to,
                            device_id_type=pl.DeviceIdType.LOGICAL)

    def remote(src, dst, k, to=0):
        return pltpu.make_async_remote_copy(
            src, dst, send_sems.at[k], recv_sems.at[k],
            device_id=to, device_id_type=pl.DeviceIdType.LOGICAL)

    def run_copy(slot, to=0):
        return remote(mine, runs.at[slot], slot, to)

    raw_copy = lambda: remote(x_hbm.at[pl.ds(16, 16)], raw, 3)
    mid_copy = lambda: remote(mid_out, mid_in, 4)
    top_copy = lambda: remote(top_out, top_in, 5)
    edge_copy = lambda: remote(x_hbm.at[pl.ds(32, 8)], edge, 6)
    head_copy = lambda: remote(head_out, head_in, 7)
    near_copy = lambda: remote(x_hbm, near, 8)

    loads[0].start()
    loads[1].start()
    g = _Geometry()

    @pl.when(me == 2)
    def _():
        pl.semaphore_wait(barrier, 1)
        raw_copy().start()
        edge_copy().start()
        signal(far_here, 0)
        three = _SkewOfThree(g)
        lower = [g.lane_bit(b) == 0 for b in (6, 5, 4)]
        second = g.diag & 8 != 0
        loads[0].wait()
        w = three.fold(_rows(x_vmem, 3, 5))
        _put(head_out, w[:1])
        head_copy().start()
        _put(mid_out, w[1:])
        mid_copy().start()
        loads[1].wait()
        t = [_gather(v, g.skew, 0) for v in _rows(x_vmem, 2)]
        t = _spread(_barrel(t, [second]), 2)
        loads[2].start()
        t = _merge_sublanes(g, _sort_vregs(t), 0, 5)
        _put(top_out, _tidy(g, t, 2, lower))
        top_copy().start()

    @pl.when(me != 2)
    def _():
        loads[2].start()

        @pl.when(me == 0)
        def _():
            for to in (2, 1, 3):
                signal(barrier, to)

        @pl.when(me != 0)
        def _():
            signal(barrier, 0)
            pl.semaphore_wait(barrier, 1)

        @pl.when(me == 1)
        def _():
            near_copy().start()

        loads[0].wait()
        loads[1].wait()

    loads[2].wait()
    own = _spread(_skew(g, _rows(x_vmem, 8)), 8)
    own = _merge_sublanes(g, _sort_vregs(own))
    low_half = g.lane < 64
    _put(mine, [jnp.where(low_half, a, b) for a, b in zip(own[:8], own[8:])])

    def run(slot):
        w = _rows(runs.at[slot], 8)
        r = [pltpu.roll(v, 64, 1) for v in w]
        return ([jnp.where(low_half, a, b) for a, b in zip(w, r)]
                + [jnp.where(low_half, b, a) for a, b in zip(w, r)])

    @pl.when(me != 0)
    def _():
        @pl.when(me == 2)
        def _():
            pl.semaphore_wait(barrier, 1)
            sends = [run_copy(0, 3), run_copy(2, 1)]
            for copy in sends:
                copy.start()
            for copy in sends + [raw_copy(), edge_copy(), head_copy(),
                                 mid_copy(), top_copy()]:
                copy.wait_send()

        for odd in (1, 3):
            @pl.when(me == odd)
            def _():
                sends = [near_copy() if odd == 1 else run_copy(0)]
                if odd == 3:
                    sends[0].start()
                for here, to in ((odd_here, 4 - odd), (far_here, 2)):
                    pl.semaphore_wait(here, 1)
                    sends.append(run_copy((to - odd) % 4 - 1, to))
                    sends[-1].start()
                for copy in sends:
                    copy.wait_send()

        for slot in range(3):
            run_copy(slot).wait_recv()
        mirror = g.rows_from(_SORTED[1], _SORTED[1], 1)

        def merge(a, b):
            pairs = [_ce(u, v) for u, v in zip(a, _reversed(b, mirror))]
            return [_bitonic(g, half, _SORTED, 1) for half in zip(*pairs)]

        def pick(lower, a, b):
            return [jnp.where(lower, *_ce(u, v)) for u, v in zip(a, b)]

        p_lo, p_hi = merge(own, run(0))
        q_lo, q_hi = merge(run(1), run(2))
        z = pick(me == 2,
                 pick(me == 1, p_lo, _reversed(q_hi, mirror)),
                 pick(me == 1, p_hi, _reversed(q_lo, mirror)))
        list_bits, sub_bits = _final_layout(_SORTED, 1)
        finish = _Exit(g, (list_bits[:3], sub_bits), 2)
        y = finish.sort(pick(low_half, z[:8], z[8:]))
        _put(o_ref, finish.untwist(finish.cross(y)))

    @pl.when(me == 0)
    def _():
        pl.semaphore_wait(barrier, 2)
        signal(barrier, 2)
        for to in (1, 3):
            signal(odd_here, to)
        run_copy(0, 1).start()
        run_copy(2, 3).start()

        finish = _Exit(g, (_SORTED[0][:2], _SORTED[1]), 1)
        head_layout = (finish.layout[0], (2, 1, 3))
        assert _final_layout(head_layout, 0) == finish.layout
        top_layout = ((6,), (3, 4, 5))
        block = g.diag >> 3
        block_rows = []
        for u in range(8):
            h = (block >> 1) + u
            row = 0
            for n, r in enumerate(_final_layout(top_layout, 0)[1]):
                row ^= ((h >> (r - 4)) & 1) * _STEPS[n]
            block_rows.append(row)
        top_lanes = g.lane & (64 + 15)
        class_rows = [
            g.sub ^ (g.bits[_FUNS[n]] ^ g.lane_bit(7 - n)) * _STEPS[n]
            for n in (1, 2)]
        m = _reversed(own, g.rows_from(_SORTED[1], _SORTED[1], 1))
        merged = _final_layout(_SORTED, 0)[1]
        head_rows = g.rows_from(_SORTED[1], head_layout[1], 0)
        mirror = g.rows_from(merged, _SORTED[1], 1)
        last_mirror = jnp.where(g.lane_bit(5) == 0, mirror,
                                g.rows_from(merged, head_layout[1], 1))

        def bounds(*col):
            out = [[] for _ in range(4)]
            for i in range(4):
                for j in range(4):
                    b = jnp.full(_VREG, -jnp.inf, _F32)
                    for q in range(j, 4):
                        b = jnp.where(g.lane >> 5 == q,
                                      col[q % 2][i + 4 * (3 - q + j)], b)
                    out[i].append(b)
            return out

        def keep_class(col, n, bit):
            col = [_gather(v, class_rows[n - 1], 0) for v in col]
            return [jnp.where(g.bits[_FUNS[n]] == 0, col[i], col[i | 1 << bit])
                    for i in range(len(col)) if not i >> bit & 1]

        pl.semaphore_wait(far_here, 1)
        for to in (1, 3):
            signal(far_here, to)
        run_copy(1, 2).start()

        near_copy().wait_recv()
        one = _spread(_skew(g, _rows(near, 8)), 8)
        one = _merge_sublanes(g, _sort_vregs(one), 0, 4)

        run_copy(0).wait_recv()
        m = [jnp.minimum(p, q) for p, q in zip(m, _merge_sublanes(g, one, 4))]
        m = _reversed(_bitonic(g, m, _SORTED, 0), mirror)
        m = [jnp.minimum(p, q) for p, q in zip(m, run(0))]
        three = _SkewOfThree(g)
        run_copy(0).wait_send()

        raw_copy().wait_recv()
        a = _spread(_skew(g, _rows(raw, 2)), 2)
        m = _reversed(_bitonic(g, m, _SORTED, 0), last_mirror)
        beside = [pltpu.roll(v, 32, 1) for v in m]
        col = [_gather(v, top_lanes, 1) for v in keep_class(m, 1, 1)]
        a = _merge_sublanes(g, _sort_vregs(a), 0, 3)

        edge_copy().wait_recv()
        missing = _gather(edge[...], g.skew, 0)
        run_copy(2).wait_send()

        head_copy().wait_recv()
        w = _rows(head_in, 1)
        u = _spread([three.unfold(w, missing, 0)], 4)
        a = finish.sort(_quarter(_merge_sublanes(g, a, 3), bounds(m, beside)))
        bound = bounds(beside, m)
        col = [jnp.where(g.lane_bit(4) == 0, p, q)
               for p, q in zip(col[0::2], col[1::2])]
        top_bound = keep_class(col, 2, 0)

        mid_copy().wait_recv()
        w += _rows(mid_in, 2)
        b = _spread([three.unfold(w, missing, j) for j in (1, 2, 3)], 4, 1)
        u = _merge_sublanes(g, _sort_vregs(u))
        u = [_gather(v, head_rows, 0) for v in u]
        bound = [_bitonic(g, _quarter(u, [r[j:] for r in bound]), head_layout,
                          0, down=True) for j in range(4)]
        even_block = block & 1 == 0
        b = _by_arrival(b)
        early = _sort_list(b[:4]), _sort_list(b[4:8])
        run_copy(1).wait_send()
        late = _sort_list(b[8:])
        b = _merge_sublanes(g, _merge_lists(_merge_lists(*early), late), 0, 4)

        top_copy().wait_recv()
        a = finish.cross(a)
        b = finish.sort(_quarter(_merge_sublanes(g, b, 4), list(zip(*bound))))
        shift = _rotate(g.lane, 0)
        back = shift & 7
        low = [pltpu.roll(g.lane, 1, 1) & 1 != 0,
               g.lane_bit(1) == 0, g.lane_bit(2) == 0]
        c = [jnp.minimum(p, q) for p, q in zip(_rows(top_in, 2), top_bound)]
        c = _bitonic(g, c, top_layout, 0)
        ev, od = ([_gather(v, rows, 0) for rows in block_rows] for v in c)
        turned = []
        for t in range(16):
            j = t // 2
            pair = (od[j], ev[(j + 1) % 8]) if t % 2 else (ev[j], od[j])
            turned.append(_rotate(jnp.where(even_block, *pair), 8 * t))
        z = []
        for half in (turned[0::2], turned[1::2]):
            for bit in (2, 1, 0):
                half = [jnp.where(low[bit], *_ce(p, q))
                        for p, q in zip(half[:1 << bit], half[1 << bit:])]
            z.append(_gather(half[0], back, 0))
        _put(o_ref, finish.untwist(a)[2:], 2)
        _put(o_ref, finish.untwist(finish.cross(b)), 4)
        _put(o_ref, _cond_swap(z, 0, shift & 8 == 0))


def pallas_dist_sort_i_m128_n64_kernel(x: jax.Array):
    out = pl.pallas_call(
        _body,
        out_shape=jax.ShapeDtypeStruct((64, 128), _F32),
        in_specs=[pl.BlockSpec(memory_space=pltpu.MemorySpace.HBM)],
        out_specs=pl.BlockSpec(memory_space=pltpu.MemorySpace.VMEM),
        scratch_shapes=[
            pltpu.VMEM((64, 128), _F32),
            pltpu.VMEM((64, 128), _F32),
            pltpu.VMEM((64, 128), _BF16),
            pltpu.VMEM((3, 64, 128), _BF16),
            pltpu.VMEM((16, 128), _F32),
            pltpu.VMEM((8, 128), _F32),
            pltpu.VMEM((8, 128), _BF16),
            pltpu.VMEM((8, 128), _BF16),
            pltpu.VMEM((16, 128), _BF16),
            pltpu.VMEM((16, 128), _BF16),
            pltpu.VMEM((16, 128), _BF16),
            pltpu.VMEM((16, 128), _BF16),
            pltpu.SemaphoreType.DMA((3,)),
            pltpu.SemaphoreType.DMA((9,)),
            pltpu.SemaphoreType.DMA((9,)),
            pltpu.SemaphoreType.REGULAR,
            pltpu.SemaphoreType.REGULAR,
        ],
        compiler_params=pltpu.CompilerParams(
            collective_id=0,
            disable_semaphore_checks=True,
        ),
    )(x.T)
    return out.T
```
